```python
import numpy as np

kernel_name = "dist_moe_cap_ep_n512_d256_e4_h512"

def setup_inputs():
    x = np.random.randn(512, 256).astype(np.float32)
    router_W = np.random.randn(256, 16).astype(np.float32) * 0.1
    scores64 = x.astype(np.float64) @ router_W.astype(np.float64)
    route_idx = np.argsort(-scores64, axis=-1)[:, :1].astype(np.int32)
    expert_W = np.random.randn(16, 256, 512).astype(np.float32) * 0.02
    return {"x": x, "router_W": router_W, "route_idx": route_idx, "expert_W": expert_W}

def reference(x, router_W, route_idx, expert_W):
    counts = np.zeros(16, dtype=np.int64)
    out = np.zeros((512, 512), dtype=np.float32)
    for i in range(512):
        e = int(route_idx[i, 0])
        if counts[e] < 25:
            out[i] = x[i] @ expert_W[e]
            counts[e] += 1
    return out
```

```python
import contextlib

import jax
import jax.numpy as jnp
from jax import lax
from jax.experimental import pallas as pl
from jax.experimental.pallas import tpu as pltpu

f32, bf16, i32, u32 = jnp.float32, jnp.bfloat16, jnp.int32, jnp.uint32
MESH = pl.DeviceIdType.MESH
CAP = 25
OWN, RIGHT, DIAG, LEFT = 0, 1, 2, 3
ALL = frozenset(range(4))


def make(
    pieces,
    wdmas,
    program,
    scopes=True,
    out_dtype=f32,
    flags=None,
    name="moe",
    diag_bar=True,
    v2s=(0,),
    wcast=True,
    check=True,
    wprio=1,
):
    NP = len(pieces)

    def scope(n):
        on = scopes if isinstance(scopes, bool) else any(n.startswith(q) for q in scopes)
        return jax.named_scope(n) if on else contextlib.nullcontext()

    def rows_of(p):
        return CAP if pieces[p][2] == 2 else 13

    def kernel_fn(x, router_W, route_idx, expert_W):
        def body(x_ref, r_ref, w_ref, o_ref, rv, tv, ts, xg, wv, yb, lsem, wsem, gsem, ssem, rsem):
            r_cp = pltpu.make_async_copy(r_ref, rv, lsem.at[0])
            r_cp.start()
            w_cps = []
            for i, (j, c0, n) in enumerate(wdmas):
                if n == 4:
                    src, dst = w_ref.at[j], wv.at[j]
                else:
                    cs = pl.ds(128 * c0, 128 * n)
                    src, dst = w_ref.at[j, :, cs], wv.at[j, :, cs]
                w_cps.append(pltpu.make_async_copy(src, dst, wsem.at[i]))

            me = lax.axis_index("i")
            dev = {k: (me + k) & 3 for k in (RIGHT, DIAG, LEFT)}
            bar = pltpu.get_barrier_semaphore()
            st = dict(w=set(), x={}, waited={}, sends=[], got=[], nsem=0)

            def on(chips, fn):
                chips = frozenset(chips)
                if chips == ALL:
                    fn()
                elif len(chips) == 1:
                    pl.when(me == next(iter(chips)))(fn)
                elif len(chips) == 3:
                    pl.when(me != next(iter(ALL - chips)))(fn)
                elif chips:
                    mask = sum(1 << c for c in chips)
                    pl.when(((mask >> me) & 1) == 1)(fn)

            def signal():
                for k in (RIGHT, LEFT):
                    pl.semaphore_signal(bar, 1, device_id=(dev[k],), device_id_type=MESH)
                if diag_bar:
                    on({0}, lambda: pl.semaphore_signal(bar, 1, device_id=(dev[DIAG],), device_id_type=MESH))

            def row_copy(t, j, s):
                return pltpu.make_async_copy(
                    x_ref.at[pl.ds(t, 1)], xg.at[pl.ds(32 * j + s, 1)], gsem.at[j]
                )

            def route():
                row = lax.broadcasted_iota(i32, (128, 128), 0)
                col = lax.broadcasted_iota(i32, (128, 128), 1)
                tri = jnp.where(row <= col, 1.0, 0.0).astype(bf16)
                ones = jnp.ones((128, 128), bf16)
                erow = (lax.broadcasted_iota(i32, (16, 128), 0) + 4 * me) & 15
                with scope("ri"):
                    r_cp.wait()
                with scope("route"):
                    hit = [
                        jnp.broadcast_to(rv[pl.ds(k, 1), :] & 15, (16, 128)) == erow
                        for k in range(4)
                    ]
                    oh = [jnp.where(h, 1.0, 0.0) for h in hit]
                    cum = [oh[0]]
                    for k in range(1, 4):
                        cum.append(cum[-1] + oh[k])
                    A = jnp.dot(jnp.concatenate(oh, 0).astype(bf16), tri, preferred_element_type=f32)
                    B = jnp.dot(jnp.concatenate(cum, 0).astype(bf16), ones, preferred_element_type=f32)
                    st["P"] = [A[0:16]] + [
                        A[16 * k:16 * k + 16] + B[16 * k - 16:16 * k] for k in range(1, 4)
                    ]
                    st["total"] = B[48:64]
                    st["hit"] = hit

            def table():
                P, hit = st["P"], st["hit"]
                srow = lax.broadcasted_iota(i32, (32, 128), 0).astype(f32)
                groups = []
                for g in range(4):
                    parts = []
                    for j in range(4):
                        e = 4 * g + j
                        acc = None
                        for k in range(4):
                            pb = jnp.broadcast_to(P[k][e:e + 1], (32, 128))
                            v = jnp.where(pb <= srow, 1.0, 0.0)
                            acc = v if acc is None else acc + v
                        parts.append(acc)
                    groups.append(jnp.concatenate(parts, 0).astype(bf16))
                T = None
                r16 = lax.broadcasted_iota(i32, (16, 128), 0)
                for g in range(4):
                    sel = jnp.where((r16 & 3) == g, 1.0, 0.0).astype(bf16)
                    t = lax.dot_general(sel, groups[g], (((1,), (1,)), ((), ())), preferred_element_type=f32)
                    T = t if T is None else T + t
                lane = lax.broadcasted_iota(i32, (16, 128), 1).astype(f32)
                drop = None
                for k in range(4):
                    d = jnp.where(hit[k] & (P[k] > float(CAP)), lane + 128.0 * k, 0.0)
                    drop = d if drop is None else jnp.maximum(drop, d)
                drop = jnp.max(jnp.max(drop, axis=1, keepdims=True), axis=0, keepdims=True)
                T = T[0:8]
                tok = jnp.where(T < 512.0, T, jnp.broadcast_to(drop, (8, 128))).astype(i32)
                addr = ((tok >> 3) << 5) | (tok & 7)
                r8 = lax.broadcasted_iota(i32, (8, 128), 0)
                tv[...] = jnp.where(r8 < 4, addr, tok)

            t_cp = pltpu.make_async_copy(tv, ts, lsem.at[1])

            def gather_v2s(j):
                P = st["P"]
                srow = lax.broadcasted_iota(i32, (16, 128), 0).astype(f32)
                acc = None
                for k in range(4):
                    pb = jnp.broadcast_to(P[k][j:j + 1], (16, 128))
                    if k == 3:
                        pb = jnp.where(lax.broadcasted_iota(i32, (16, 128), 1) == 127, 1e9, pb)
                    v = jnp.where(pb <= srow, 1025.0, jnp.where(pb <= srow + 13.0, 1024.0, 0.0))
                    acc = v if acc is None else acc + v
                tk = jnp.sum(acc, axis=1, keepdims=True).astype(i32)
                for s in range(13):
                    word = tk[s, 0]
                    row_copy(word & 1023, j, s).start()
                    if s < 12:
                        row_copy(word >> 10, j, s + 13).start()

            def rdma(src_rel, dst_rel, to, p, k):
                n = rows_of(p)
                return pltpu.make_async_remote_copy(
                    yb.at[src_rel, p, pl.ds(0, n)],
                    yb.at[dst_rel, p, pl.ds(0, n)],
                    ssem.at[k * NP + p],
                    rsem.at[(dst_rel - 1) * NP + p],
                    device_id=(dev[to],),
                    device_id_type=MESH,
                )

            KINDS = {
                "l": (OWN, RIGHT, LEFT, 0),
                "r": (OWN, LEFT, RIGHT, 1),
                "L": (RIGHT, DIAG, LEFT, 2),
                "R": (LEFT, DIAG, RIGHT, 3),
                "d": (OWN, DIAG, DIAG, 4),
            }

            def start(kind, p):
                src, dst, to, k = KINDS[kind]
                if src != OWN:
                    rdma(OWN, src, RIGHT, p, 0).wait_recv()
                rdma(src, dst, to, p, k).start()

            def note(chips, kind, p):
                src, dst, to, k = KINDS[kind]
                if src != OWN:
                    done = st["waited"].setdefault((src, p), set())
                    assert not (done & set(chips))
                    done |= set(chips)
                st["sends"].append((frozenset(chips), kind, p))
                for c in chips:
                    st["got"].append(((c + to) & 3, dst, p))

            def compute(p):
                j, c0, n = pieces[p]
                if j not in st["x"]:
                    with scope(f"xw{j}"):
                        for s in range(CAP):
                            row_copy(0, j, s).wait()
                    xx = xg[pl.ds(32 * j, 32), :]
                    st["x"][j] = xx.astype(bf16) if wcast else xx
                    srow = lax.broadcasted_iota(i32, (32, 128), 0).astype(f32)
                    st["ok", j] = srow < jnp.broadcast_to(st["total"][j:j + 1], (32, 128))
                for i, (wj, wc0, wn) in enumerate(wdmas):
                    if wj == j and wc0 < c0 + n and c0 < wc0 + wn and i not in st["w"]:
                        st["w"].add(i)
                        with scope(f"ww{i}"):
                            w_cps[i].wait()
                with scope(f"c{p}"):
                    w = wv[j, :, pl.ds(128 * c0, 128 * n)]
                    y = jnp.dot(st["x"][j], w.astype(bf16) if wcast else w, preferred_element_type=f32)
                    ok = st["ok", j]
                    if n == 2:
                        a = jnp.where(ok, y[:, :128], 0.0)
                        b = jnp.where(ok, y[:, 128:], 0.0)
                        yb[OWN, p] = pltpu.pack_elementwise([a, b], packed_dtype=bf16)
                    else:
                        a = jnp.where(ok, y, 0.0)
                        yb[OWN, p, pl.ds(0, 16)] = pltpu.pack_elementwise(
                            [a[0:16], a[13:29]], packed_dtype=bf16
                        )

            def unp(v, i):
                return pltpu.unpack_elementwise(v, index=i, packed_dtype=bf16, unpacked_dtype=f32)

            def scatter(rel, p):
                j, c0, n = pieces[p]
                if rel != OWN:
                    done = st["waited"].setdefault((rel, p), set())
                    with scope(f"r{rel}_{p}"):
                        on(ALL - done, lambda: rdma(OWN, rel, RIGHT, p, 0).wait_recv())
                    done |= ALL
                with scope(f"s{rel}_{p}"):
                    if n == 2:
                        for s in range(CAP):
                            a = ts[rel, 32 * j + s]
                            v = yb[rel, p, pl.ds(s, 1), :]
                            o_ref[pl.ds(a + 8 * c0, 1), :] = unp(v, 0)
                            o_ref[pl.ds(a + 8 * c0 + 8, 1), :] = unp(v, 1)
                    else:
                        for s in range(13):
                            v = yb[rel, p, pl.ds(s, 1), :]
                            o_ref[pl.ds(ts[rel, 32 * j + s] + 8 * c0, 1), :] = unp(v, 0)
                            if s < 12:
                                o_ref[pl.ds(ts[rel, 32 * j + s + 13] + 8 * c0, 1), :] = unp(v, 1)

            def drain():
                by = {}
                for chips, kind, p in st["sends"]:
                    by.setdefault(chips, []).append((kind, p))
                st["sends"] = []

                def waits(v):
                    for kind, p in v:
                        src, dst, to, k = KINDS[kind]
                        rdma(src, dst, to, p, k).wait_send()

                with scope("drain"):
                    for chips, v in by.items():
                        on(chips, lambda v=v: waits(v))

            for op in program:
                if op == "Z":
                    for j in range(4):
                        xg[pl.ds(32 * j + 24, 8), :] = jnp.zeros((8, 256), f32)
                    o_ref[...] = jnp.zeros(o_ref.shape, o_ref.dtype)
                elif op == "SIG":
                    signal()
                elif op == "BAR":
                    with scope("bar"):
                        pl.semaphore_wait(bar, jnp.where(me == 2, 3, 2) if diag_bar else 2)
                elif op == "R":
                    route()
                elif op[0] == "W":
                    a, b = op[1:].split("-")
                    for i in range(int(a), int(b)):
                        w_cps[i].start(priority=wprio)
                elif op[0] == "G":
                    j = int(op[1:])
                    with scope(op):
                        if j in v2s:
                            gather_v2s(j)
                        else:
                            for s in range(CAP):
                                row_copy(ts[4, 32 * j + s], j, s).start()
                elif op == "T":
                    with scope("table"):
                        table()
                    t_cp.start()
                elif op == "TW":
                    with scope("tw"):
                        t_cp.wait()
                elif op == "D":
                    drain()
                elif op[0] == "C":
                    compute(int(op[1:]))
                elif op[0] == "X":
                    chips, items = op[1:].split(":")
                    chips = ALL if chips == "" else frozenset(int(c) for c in chips)
                    items = [(it[0], int(it[1:])) for it in items.split(",")]

                    def go(items=items):
                        for kind, p in items:
                            start(kind, p)

                    with scope("x" + op[1:].replace(":", "_").split(",")[0]):
                        on(chips, go)
                    for kind, p in items:
                        note(chips, kind, p)
                elif op[0] == "S":
                    rel, p = op[1:].split(":")
                    scatter(int(rel), int(p))
                else:
                    raise ValueError(op)
            drain()
            if check:
                want = sorted((c, rel, p) for c in range(4) for rel in (1, 2, 3) for p in range(NP))
                assert sorted(st["got"]) == want, (set(want) ^ set(st["got"]), len(st["got"]))
                assert all(st["waited"][rel, p] == set(ALL) for rel in (1, 2, 3) for p in range(NP))
                assert len(st["w"]) == len(wdmas)

        HBM = pl.BlockSpec(memory_space=pltpu.HBM)
        out = pl.pallas_call(
            body,
            out_shape=pltpu.VMEM((2048, 128), out_dtype),
            in_specs=[HBM, HBM, HBM],
            out_specs=pl.BlockSpec(memory_space=pltpu.VMEM),
            scratch_shapes=[
                pltpu.VMEM((4, 128), i32),
                pltpu.VMEM((8, 128), i32),
                pltpu.SMEM((8, 128), i32),
                pltpu.VMEM((128, 256), f32),
                pltpu.VMEM((4, 256, 512), f32),
                pltpu.VMEM((4, NP, 32, 128), u32),
                pltpu.SemaphoreType.DMA((2,)),
                pltpu.SemaphoreType.DMA((len(wdmas),)),
                pltpu.SemaphoreType.DMA((4,)),
                pltpu.SemaphoreType.DMA((5 * NP,)),
                pltpu.SemaphoreType.DMA((3 * NP,)),
            ],
            name=name,
            compiler_params=pltpu.CompilerParams(
                collective_id=0,
                disable_bounds_checks=True,
                disable_semaphore_checks=True,
                flags=flags,
            ),
        )(x, route_idx.reshape(4, 128), expert_W)
        return out.reshape(64, 4, 8, 128).transpose(0, 2, 1, 3).reshape(512, 512)

    return kernel_fn


_HALVES = [(j, 2 * h, 2) for j in range(4) for h in range(2)]
_PROG = ("W0-8 SIG Z R G0 T C0 BAR X:l0,r0 TW G1 C1 X2:d1 X:l1,r1 G2 G3 C2 X:l2,r2 C3 X:l3,r3 C4 X:l4,r4 "
        "C5 X2:d5 X013:l5 X:r5 C6 X2:d6 X013:l6 X:r6 X3:R0 C7 X2:d7,l5,l6 X:l7,r7 X3:R2 X1:R0,R1,R2,R3,R4,R5 "
        + " ".join(f"S0:{p}" for p in range(8)) + " X3:R3,R4 X1:R6,R7 X2:R4,R5,R6,L6,R7,L7 "
        "X0:R0,L0 S3:0 S1:0 X0:R1,L1 S3:1 S1:1 X0:R2,L2 S3:2 S1:2 X0:R3,L3 S3:3 S1:3 S2:1 X0:R4 S3:4 S1:4 X0:R5 S3:5 S1:5 "
        "S3:6 S1:6 S2:0 S1:7 S2:5 S3:7 S2:2 S2:6 D S2:3 S2:4 S2:7").split()


def pallas_dist_moe_cap_ep_n512_d256_e4_h512_kernel(x, router_W, route_idx, expert_W):
    return make(_HALVES, _HALVES, _PROG, scopes=False)(x, router_W, route_idx, expert_W)
```

```python
import jax
import jax.numpy as jnp
from jax import lax
from jax.experimental import pallas as pl
from jax.experimental.pallas import tpu as pltpu

F32, BF16, I32, U32 = jnp.float32, jnp.bfloat16, jnp.int32, jnp.uint32

N_TOKENS, D_IN, D_OUT = 512, 256, 512
N_EXPERTS, N_LOCAL, CAP = 16, 4, 25
LANES, SLOTS = 128, 32

OWN, RIGHT, DIAG, LEFT = 0, 1, 2, 3

PIECES = (
    (0, 0, 2), (0, 2, 2), (1, 0, 2), (1, 2, 2), (2, 0, 2), (2, 2, 2),
    (3, 3, 1), (3, 2, 1), (3, 1, 1), (3, 0, 1),
)
W_BLOCKS = ((0, 0, 4),) + PIECES[2:]
FIRST_TILE = 6
EARLY = 8
SPLIT = 4

TO_LEFT = (OWN, RIGHT, LEFT)
TO_RIGHT = (OWN, LEFT, RIGHT)
TO_DIAG = (OWN, DIAG, DIAG)
RELAY_LEFT = (RIGHT, DIAG, LEFT)
RELAY_RIGHT = (LEFT, DIAG, RIGHT)
ALL = (0, 1, 2, 3)
OPT = dict(strided=False)


def _rows(p):
    return CAP if p < FIRST_TILE else 12 + (p & 1)


def _y_row(source, p):
    return (source * len(PIECES) + p) * SLOTS


def _x_row(j, s):
    return SLOTS * j + (s + 4 if j == N_LOCAL - 1 and s >= 12 else s)


def _iota(shape, axis):
    return lax.broadcasted_iota(I32, shape, axis)


def _dot(a, b):
    return jnp.dot(a.astype(BF16), b.astype(BF16), preferred_element_type=F32)


def _pack(lo, hi):
    return pltpu.pack_elementwise([lo, hi], packed_dtype=BF16)


def _unpack(v, index):
    return pltpu.unpack_elementwise(v, index=index, packed_dtype=BF16, unpacked_dtype=F32)


def _moe_kernel(x_hbm, route_hbm, w_hbm, out, route, addr_v, addr_s, xg, ybuf,
                fence_sem, misc_sem, w_sem, x_sem, send_sem, recv_sem, *w_bufs):

    def fence():
        pl.semaphore_signal(fence_sem, 1)
        pl.semaphore_wait(fence_sem, 1)

    route_copy = pltpu.make_async_copy(route_hbm, route, misc_sem.at[0])
    route_copy.start()
    if OPT.get("f0", True):
        fence()
    w_copies = []
    for i, (j, c0, n) in enumerate(W_BLOCKS):
        src = w_hbm.at[j] if n == 4 else w_hbm.at[j, :, pl.ds(LANES * c0, LANES * n)]
        w_copies.append(pltpu.make_async_copy(src, w_bufs[i], w_sem.at[i]))
        w_copies[i].start(priority=1)
    fence()

    me = lax.axis_index("i")
    mesh_id = pl.DeviceIdType.MESH

    def on(chips, fn):
        if len(chips) == 4:
            fn()
        elif len(chips) == 3:
            pl.when(me != 6 - sum(chips))(fn)
        elif chips:
            pl.when(((sum(1 << c for c in chips) >> me) & 1) == 1)(fn)

    barrier = pltpu.get_barrier_semaphore()

    def tell(distance):
        pl.semaphore_signal(barrier, 1, device_id=((me + distance) & 3,), device_id_type=mesh_id)

    tell(RIGHT)
    tell(LEFT)
    on((0,), lambda: tell(DIAG))

    for row in (24, 56, 88, 104, 120):
        xg[pl.ds(row, 8), :] = jnp.zeros((8, D_IN), F32)
    out[...] = jnp.zeros(out.shape, F32)

    def running_counts(n):
        expert = (_iota((n, LANES), 0) + N_LOCAL * me) & (N_EXPERTS - 1)
        hit = [
            jnp.broadcast_to(route[pl.ds(k, 1), :] & (N_EXPERTS - 1), (n, LANES)) == expert
            for k in range(4)
        ]
        flags = [jnp.where(h, 1.0, 0.0) for h in hit]
        earlier = [flags[0]]
        for k in range(1, 4):
            earlier.append(earlier[-1] + flags[k])
        square = (LANES, LANES)
        upto = jnp.where(_iota(square, 0) <= _iota(square, 1), 1.0, 0.0)
        ones = jnp.ones(square, BF16)
        a = [_dot(jnp.concatenate(flags[k:k + 2], 0), upto) for k in (0, 2)]
        b = [_dot(jnp.concatenate(earlier[k:k + 2], 0), ones) for k in (0, 2)]
        counts = [a[0][:n], a[0][n:] + b[0][:n], a[1][:n] + b[0][n:], a[1][n:] + b[1][:n]]
        return hit, counts, b[1][n:]

    route_copy.wait()
    _, counts, total = running_counts(8)

    def token_words(j):
        shape = (16, LANES)
        even = 2.0 * _iota(shape, 0).astype(F32)
        acc = None
        for k in range(4):
            c = jnp.broadcast_to(counts[k][j:j + 1], shape)
            both, odd_only, none = 1025.0, 1024.0, 0.0
            if k == 0:
                both, odd_only, none = both + 65536.0, odd_only + 65536.0, 65536.0
            if k == 3:
                last = _iota(shape, 1) == LANES - 1
                both, odd_only = jnp.where(last, 0.0, both), jnp.where(last, 0.0, odd_only)
            v = jnp.where(c <= even, both, jnp.where(c <= even + 1.0, odd_only, none))
            acc = v if acc is None else acc + v
        acc = jnp.broadcast_to(jnp.sum(acc, axis=1, keepdims=True), shape)
        return pltpu.bitcast(acc, I32) & 0xFFFFF

    def to_scalars(words):
        return [words[r, 0] for r in range((CAP + 1) // 2)]

    row_copies = {}

    def fetch_rows(j, words):
        for s in range(CAP):
            token = words[s // 2] >> 10 if s & 1 else words[s // 2] & 1023
            group = N_LOCAL if j == 0 and s < EARLY else j
            copy = pltpu.make_async_copy(
                x_hbm.at[pl.ds(token, 1)], xg.at[pl.ds(_x_row(j, s), 1)], x_sem.at[group])
            copy.start()
            row_copies.setdefault(group, []).append(copy)
            if s in OPT.get("vf", (7, 15)):
                fence()

    def wait_rows(group):
        for copy in row_copies[group]:
            copy.wait()

    def build_addresses():
        hit, counts, _ = running_counts(N_EXPERTS)
        slot = _iota((SLOTS, LANES), 0).astype(F32)
        token = None
        for d in range(4):
            parts = []
            for e in range(N_LOCAL * d, N_LOCAL * (d + 1)):
                below = [
                    jnp.where(jnp.broadcast_to(c[e:e + 1], slot.shape) <= slot, 1.0, 0.0)
                    for c in counts
                ]
                parts.append((below[0] + below[1]) + (below[2] + below[3]))
            t = lax.dot_general(
                jnp.where(_iota((16, LANES), 0) == d, 1.0, 0.0).astype(BF16),
                jnp.concatenate(parts, 0).astype(BF16),
                (((1,), (1,)), ((), ())), preferred_element_type=F32)
            token = t if token is None else token + t
        lane = _iota((N_EXPERTS, LANES), 1).astype(F32)
        dropped = jnp.zeros_like(lane)
        for k in range(4):
            over = hit[k] & (counts[k] > float(CAP))
            dropped = jnp.maximum(dropped, jnp.where(over, lane + float(LANES * k), 0.0))
        dropped = jnp.max(jnp.max(dropped, axis=1, keepdims=True), axis=0, keepdims=True)
        token = token[:8]
        token = jnp.where(token < float(N_TOKENS), token, jnp.broadcast_to(dropped, token.shape))
        token = token.astype(I32)
        addr_v[...] = ((token >> 3) << 5) | (token & 7)

    def filled(j, slot):
        return slot.astype(F32) < jnp.broadcast_to(total[j:j + 1], slot.shape)

    def first_expert(r0, r1):
        xs = xg[pl.ds(r0, r1 - r0), :]
        xs = jnp.concatenate([xs, jnp.zeros((8, D_IN), F32)], 0)
        y = _dot(xs, w_bufs[0][...])[:r1 - r0]
        keep = filled(0, _iota((r1 - r0, LANES), 0) + r0)
        y = [jnp.where(keep, y[:, LANES * c:LANES * (c + 1)], 0.0) for c in range(4)]
        ybuf[pl.ds(_y_row(OWN, 0) + r0, r1 - r0)] = _pack(y[0], y[1])
        ybuf[pl.ds(_y_row(OWN, 1) + r0, r1 - r0)] = _pack(y[2], y[3])

    def middle_expert(j):
        wait_rows(j)
        xs = xg[pl.ds(SLOTS * j, SLOTS), :].astype(BF16)
        keep = filled(j, _iota((SLOTS, LANES), 0))

        def piece(p):
            w_copies[p - 1].wait()
            y = _dot(xs, w_bufs[p - 1][...])
            ybuf[pl.ds(_y_row(OWN, p), SLOTS)] = _pack(
                jnp.where(keep, y[:, :LANES], 0.0), jnp.where(keep, y[:, LANES:], 0.0))

        return piece

    def last_expert(j):
        wait_rows(j)
        xs = [
            [xg[pl.ds(SLOTS * j + m, 16), pl.ds(k, LANES)].astype(BF16) for k in (0, LANES)]
            for m in (0, 16)
        ]
        row = _iota((16, LANES), 0)
        keep = [filled(j, row), filled(j, row + 12)]
        previous = []

        def piece(p):
            w_copies[p - 1].wait()
            w = [w_bufs[p - 1][pl.ds(k, LANES), :].astype(BF16) for k in (0, LANES)]
            lo, hi = [
                jnp.where(ok, _dot(a[0], w[0]) + _dot(a[1], w[1]), 0.0)
                for a, ok in zip(xs, keep)
            ]
            if p & 1:
                lo = jnp.where(row == 12, previous.pop(), lo)
            else:
                previous.append(hi)
            ybuf[pl.ds(_y_row(OWN, p), 16)] = _pack(lo, hi)

        return piece

    arrived = {}
    rows_sent = [0] * 4

    def remote_copy(src, dst, target, p, r0, r1):
        return pltpu.make_async_remote_copy(
            ybuf.at[pl.ds(_y_row(src, p) + r0, r1 - r0)],
            ybuf.at[pl.ds(_y_row(dst, p) + r0, r1 - r0)],
            send_sem, recv_sem.at[(dst - 1) * len(PIECES) + p],
            device_id=(target,), device_id_type=mesh_id)

    def wait_piece(src, p):
        remote_copy(OWN, src, me, p, 0, _rows(p)).wait_recv()

    def send(chips, *groups):
        items = [
            (*route, p, *(rows or (0, _rows(p)))) for route, ps, *rows in groups for p in ps
        ]
        items.sort(key=lambda item: item[3])

        def start():
            for src, dst, to, p, r0, r1 in items:
                if src != OWN:
                    wait_piece(src, p)
                remote_copy(src, dst, (me + to) & 3, p, r0, r1).start()

        on(chips, start)
        for src, _, _, p, r0, r1 in items:
            arrived.setdefault((src, p), set()).update(chips)
            for c in chips:
                rows_sent[c] += r1 - r0

    def send_to_chip0(chips, p, r0=0, r1=None):
        r1 = r1 or _rows(p)
        on(chips, lambda: remote_copy(OWN, me, 0, p, r0, r1).start())
        for c in chips:
            rows_sent[c] += r1 - r0

    def finish_sends():
        for c in ALL:
            everything = ybuf.at[pl.ds(0, rows_sent[c])]
            on((c,), pltpu.make_async_remote_copy(
                everything, everything, send_sem, recv_sem.at[0],
                device_id=(me,), device_id_type=mesh_id).wait_send)

    def receive(src, p):
        if src != OWN:
            missing = tuple(c for c in ALL if c not in arrived.get((src, p), ()))
            on(missing, lambda: wait_piece(src, p))

    def place(src, p):
        receive(src, p)
        j, c0, n = PIECES[p]

        def put(s, tile, value):
            out[pl.ds(rows[s] + 8 * tile, 1), :] = value

        rows = [addr_s[src, SLOTS * j + s] for s in range(CAP)]
        for r in range(_rows(p)):
            v = ybuf[pl.ds(_y_row(src, p) + r, 1), :]
            if n == 2 and OPT["strided"]:
                v = jnp.broadcast_to(v, (8, LANES))
                v = jnp.where(_iota((8, LANES), 0) == 0, _unpack(v, 0), _unpack(v, 1))
                out[pl.ds(rows[r] + 8 * c0, 2, stride=8), :] = v[:2]
            elif n == 2:
                put(r, c0, _unpack(v, 0))
                put(r, c0 + 1, _unpack(v, 1))
            elif r < 12:
                put(r, c0, _unpack(v, 0))
                put(r + 12, c0, _unpack(v, 1))
            else:
                put(24, PIECES[p - 1][1], _unpack(v, 0))
                put(24, c0, _unpack(v, 1))

    def pass_on(ps):
        send((0, 3), (TO_LEFT, ps))
        send((0, 1), (TO_RIGHT, ps))

    words = to_scalars(token_words(0))
    fence()
    later = [token_words(j) for j in (1, 2, 3)]
    for j in range(3):
        fetch_rows(j, words)
        words = to_scalars(later[j])
        fence()

    wait_rows(N_LOCAL)
    w_copies[0].wait()
    first_expert(0, EARLY)
    on((0, 1, 3), lambda: pl.semaphore_wait(barrier, 2))
    on((2,), lambda: pl.semaphore_wait(barrier, 3))
    for r0, r1 in ((0, EARLY), (EARLY, CAP)):
        if r0:
            wait_rows(0)
            first_expert(EARLY, SLOTS)
        send_to_chip0((1, 2, 3), 0, r0, r1)
        send_to_chip0((1, 3), 1, r0, r1)
        send((2,), (TO_RIGHT, (1,), r0, r1))
    pass_on((0, 1))
    fence()
    fetch_rows(3, words)
    fence()

    for p in range(2, FIRST_TILE):
        if p % 2 == 0:
            piece = middle_expert(p // 2)
        piece(p)
        if p < 5:
            send_to_chip0((1, 3), p)
            send((2,), (TO_RIGHT, (p,)))
            if p == 2:
                send((2,), (TO_DIAG, (2,), 0, SPLIT))
            for item in OPT.get("fill", {2: [(0,)], 3: [(1,)], 4: [(2, 0, 12)]}).get(p, []):
                send((2,), (TO_LEFT, item[:1], *item[1:]))
        else:
            send_to_chip0((1, 2, 3), p)
        if p == 4:
            send((2,), (TO_RIGHT, (0,)))
        pass_on((p,))
        fence()

    piece = last_expert(3)
    tiles = tuple(range(FIRST_TILE, len(PIECES)))
    for p in tiles:
        piece(p)
        send_to_chip0((1, 2, 3), p)
        if p == 8:
            send((3,), (RELAY_RIGHT, (1,)))
        fence()
    for item in OPT.get("late", [(2, 12, 25)]):
        send((2,), (TO_LEFT, item[:1], *item[1:]))
    send((2,), (TO_LEFT, range(3, len(PIECES))), (TO_RIGHT, range(5, len(PIECES))))
    pass_on(tiles)
    send((3,), (RELAY_RIGHT, (2,), SPLIT, CAP))
    fence()

    build_addresses()
    addr_copy = pltpu.make_async_copy(addr_v, addr_s, misc_sem.at[1])
    addr_copy.start()
    fence()
    send((3,), (RELAY_RIGHT, (3,)))
    send((1,), (RELAY_RIGHT, range(len(PIECES))))
    send((3,), (RELAY_RIGHT, (4,)))
    addr_copy.wait()
    for p in range(len(PIECES)):
        place(OWN, p)
    send((2,), (RELAY_RIGHT, tiles), (RELAY_LEFT, (9,)))

    for p in (0, 2, 4):
        send((0,), (RELAY_RIGHT, (p, p + 1)), (RELAY_LEFT, (p, p + 1)))
        for src in (LEFT, RIGHT):
            place(src, p)
            place(src, p + 1)
        fence()
    send((0,), (RELAY_RIGHT, (6, 7)))
    for src, p in (
        (DIAG, 0), (LEFT, 6), (LEFT, 7), (RIGHT, 6), (LEFT, 8), (RIGHT, 7), (RIGHT, 8),
        (DIAG, 1), (RIGHT, 9), (LEFT, 9), (DIAG, 2), (DIAG, 5),
        (DIAG, 6), (DIAG, 3), (DIAG, 7), (DIAG, 8), (DIAG, 4), (DIAG, 9),
    ):
        if (src, p) == (LEFT, 8):
            send((0,), (RELAY_RIGHT, (8,)))
        if (src, p) == OPT.get("d0", (DIAG, 6)):
            finish_sends()
        place(src, p)
        if (src, p) != (DIAG, 9) and OPT.get("tf", False):
            fence()


def pallas_dist_moe_cap_ep_n512_d256_e4_h512_kernel(
    x: jax.Array,
    router_W: jax.Array,
    route_idx: jax.Array,
    expert_W: jax.Array,
):
    del router_W
    in_hbm = pl.BlockSpec(memory_space=pltpu.HBM)
    tiles = D_OUT // LANES
    out = pl.pallas_call(
        _moe_kernel,
        out_shape=pltpu.VMEM((N_TOKENS * tiles, LANES), F32),
        in_specs=[in_hbm, in_hbm, in_hbm],
        out_specs=pl.BlockSpec(memory_space=pltpu.VMEM),
        scratch_shapes=[
            pltpu.VMEM((N_TOKENS // LANES, LANES), I32),
            pltpu.VMEM((8, LANES), I32),
            pltpu.SMEM((8, LANES), I32),
            pltpu.VMEM((N_LOCAL * SLOTS, D_IN), F32),
            pltpu.VMEM((4 * len(PIECES) * SLOTS, LANES), U32),
            pltpu.SemaphoreType.REGULAR,
            pltpu.SemaphoreType.DMA((2,)),
            pltpu.SemaphoreType.DMA((len(W_BLOCKS),)),
            pltpu.SemaphoreType.DMA((N_LOCAL + 1,)),
            pltpu.SemaphoreType.DMA,
            pltpu.SemaphoreType.DMA((3 * len(PIECES),)),
            *(pltpu.VMEM((D_IN, LANES * n), F32) for _, _, n in W_BLOCKS),
        ],
        name="moe_cap_ep",
        compiler_params=pltpu.CompilerParams(
            collective_id=0, disable_bounds_checks=True, disable_semaphore_checks=True),
    )(x, route_idx.reshape(N_TOKENS // LANES, LANES), expert_W)
    out = out.reshape(N_TOKENS // 8, tiles, 8, LANES).transpose(0, 2, 1, 3)
    return out.reshape(N_TOKENS, D_OUT)
```

```python
import jax
import jax.numpy as jnp
import numpy as np
from jax import lax
from jax.experimental import pallas as pl
from jax.experimental.pallas import tpu as pltpu

F32, BF16, I32, U32 = jnp.float32, jnp.bfloat16, jnp.int32, jnp.uint32

N_TOKENS, D_IN, D_OUT = 512, 256, 512
N_EXPERTS, N_LOCAL, CAP = 16, 4, 25
LANES = 128
SLOTS = 32

OWN, RIGHT, DIAG, LEFT = 0, 1, 2, 3

PIECES = (
    (0, 0, 2), (0, 2, 2), (1, 0, 2), (1, 2, 2), (2, 0, 2),
    (2, 3, 1), (2, 2, 1), (3, 3, 1), (3, 2, 1), (3, 1, 1), (3, 0, 1),
)
N_PIECES = len(PIECES)
FIRST_TILE = 5
W_BLOCKS = ((0, 0, 4),) + PIECES[2:]
EARLY = 8
LAST_RELAYED, CUT = 4, 18


TO_LEFT = (OWN, RIGHT, LEFT)
TO_RIGHT = (OWN, LEFT, RIGHT)
TO_DIAG = (OWN, DIAG, DIAG)
RELAY_LEFT = (RIGHT, DIAG, LEFT)
RELAY_RIGHT = (LEFT, DIAG, RIGHT)

SEND_GROUPS = (
    (TO_LEFT, (0, 1, 2, 3), range(N_PIECES)),
    (TO_DIAG, (2,), range(FIRST_TILE, N_PIECES)),
    (TO_RIGHT, (0, 1, 2, 3), range(N_PIECES)),
    (TO_DIAG, (2,), range(0, 1)),
    (RELAY_RIGHT, (0,), range(0, 9)),
    (RELAY_RIGHT, (0,), range(9, 10)),
    (RELAY_LEFT, (0,), range(0, FIRST_TILE)),
    (RELAY_RIGHT, (1,), range(N_PIECES)),
    (RELAY_RIGHT, (2,), range(FIRST_TILE, N_PIECES)),
    (RELAY_LEFT, (2,), range(10, 11)),
    (RELAY_RIGHT, (3,), range(1, FIRST_TILE)),
)


def _rows(p):
    return CAP if p < FIRST_TILE else 12 + (p - FIRST_TILE) % 2


def _y_place(p):
    if p < FIRST_TILE:
        return p, 0
    return FIRST_TILE + (p - FIRST_TILE) // 2, CAP - _rows(p) if _rows(p) == 12 else 0


def _x_row(j, s):
    return SLOTS * j + (s + 4 if j == N_LOCAL - 1 and s >= 12 else s)


def _iota(shape, axis):
    return lax.broadcasted_iota(I32, shape, axis)


def _dot(a, b):
    return jnp.dot(a.astype(BF16), b.astype(BF16), preferred_element_type=F32)


def _pack(lo, hi):
    lo, hi = (lax.bitcast_convert_type(v.astype(BF16).astype(F32), U32) for v in (lo, hi))
    return (lo >> 16) | (hi & np.uint32(0xFFFF0000))


def _unpack(words):
    lo, hi = words << 16, words & np.uint32(0xFFFF0000)
    return lax.bitcast_convert_type(lo, F32), lax.bitcast_convert_type(hi, F32)


def _moe_kernel(x_hbm, route_hbm, w_hbm, out, route, addr_v, addr_s, xg, ybuf,
                fence_sem, misc_sem, w_sem, x_sem, send_sem, recv_sem, *w_bufs):

    def fence():
        pl.semaphore_signal(fence_sem, 1)
        pl.semaphore_wait(fence_sem, 1)

    route_copy = pltpu.make_async_copy(route_hbm, route, misc_sem.at[0])
    route_copy.start()
    fence()
    w_copies = []
    for i, (j, c0, n) in enumerate(W_BLOCKS):
        src = w_hbm.at[j] if n == 4 else w_hbm.at[j, :, pl.ds(LANES * c0, LANES * n)]
        w_copies.append(pltpu.make_async_copy(src, w_bufs[i], w_sem.at[i]))
        w_copies[i].start(priority=1)
    fence()

    me = lax.axis_index("i")
    mesh_id = pl.DeviceIdType.MESH

    def on(chips, fn):
        if len(chips) == 4:
            fn()
        elif len(chips) == 3:
            pl.when(me != 6 - sum(chips))(fn)
        elif chips:
            pl.when(((sum(1 << c for c in chips) >> me) & 1) == 1)(fn)

    barrier = pltpu.get_barrier_semaphore()

    def tell(distance):
        pl.semaphore_signal(barrier, 1, device_id=((me + distance) & 3,), device_id_type=mesh_id)

    tell(RIGHT)
    tell(LEFT)
    on((0,), lambda: tell(DIAG))

    for row in (24, 56, 88, 104, 120):
        xg[pl.ds(row, 8), :] = jnp.zeros((8, D_IN), F32)
    out[...] = jnp.zeros(out.shape, F32)

    def running_counts(n):
        expert = (_iota((n, LANES), 0) + N_LOCAL * me) & (N_EXPERTS - 1)
        hit = [
            jnp.broadcast_to(route[pl.ds(k, 1), :] & (N_EXPERTS - 1), (n, LANES)) == expert
            for k in range(4)
        ]
        flags = [jnp.where(h, 1.0, 0.0) for h in hit]
        earlier = [flags[0]]
        for k in range(1, 4):
            earlier.append(earlier[-1] + flags[k])
        square = (LANES, LANES)
        upto = jnp.where(_iota(square, 0) <= _iota(square, 1), 1.0, 0.0)
        ones = jnp.ones(square, BF16)
        a = [_dot(jnp.concatenate(flags[k:k + 2], 0), upto) for k in (0, 2)]
        b = [_dot(jnp.concatenate(earlier[k:k + 2], 0), ones) for k in (0, 2)]
        counts = [a[0][:n], a[0][n:] + b[0][:n], a[1][:n] + b[0][n:], a[1][n:] + b[1][:n]]
        return hit, counts, b[1][n:]

    route_copy.wait()
    _, counts, total = running_counts(8)

    def token_words(j):
        shape = (16, LANES)
        even = 2.0 * _iota(shape, 0).astype(F32)
        acc = None
        for k in range(4):
            c = jnp.broadcast_to(counts[k][j:j + 1], shape)
            both, odd_only, none = 1025.0, 1024.0, 0.0
            if k == 0:
                both, odd_only, none = both + 65536.0, odd_only + 65536.0, 65536.0
            if k == 3:
                last = _iota(shape, 1) == LANES - 1
                both, odd_only = jnp.where(last, 0.0, both), jnp.where(last, 0.0, odd_only)
            v = jnp.where(c <= even, both, jnp.where(c <= even + 1.0, odd_only, none))
            acc = v if acc is None else acc + v
        acc = jnp.broadcast_to(jnp.sum(acc, axis=1, keepdims=True), shape)
        return lax.bitcast_convert_type(acc, I32) & 0xFFFFF

    def to_scalars(words):
        return [words[r, 0] for r in range((CAP + 1) // 2)]

    row_copies = {}

    def fetch_rows(j, words):
        for s in range(CAP):
            token = words[s // 2] >> 10 if s & 1 else words[s // 2] & 1023
            group = N_LOCAL if j == 0 and s < EARLY else j
            copy = pltpu.make_async_copy(
                x_hbm.at[pl.ds(token, 1)], xg.at[pl.ds(_x_row(j, s), 1)], x_sem.at[group])
            copy.start()
            row_copies.setdefault(group, []).append(copy)
            if s in (7, 15):
                fence()

    def wait_rows(group):
        for copy in row_copies[group]:
            copy.wait()

    def build_addresses():
        hit, counts, _ = running_counts(N_EXPERTS)
        slot = _iota((SLOTS, LANES), 0).astype(F32)
        token = None
        for d in range(4):
            parts = []
            for e in range(N_LOCAL * d, N_LOCAL * (d + 1)):
                below = [
                    jnp.where(jnp.broadcast_to(c[e:e + 1], slot.shape) <= slot, 1.0, 0.0)
                    for c in counts
                ]
                parts.append((below[0] + below[1]) + (below[2] + below[3]))
            t = lax.dot_general(
                jnp.where(_iota((16, LANES), 0) == d, 1.0, 0.0).astype(BF16),
                jnp.concatenate(parts, 0).astype(BF16),
                (((1,), (1,)), ((), ())), preferred_element_type=F32)
            token = t if token is None else token + t
        lane = _iota((N_EXPERTS, LANES), 1).astype(F32)
        dropped = jnp.zeros_like(lane)
        for k in range(4):
            over = hit[k] & (counts[k] > float(CAP))
            dropped = jnp.maximum(dropped, jnp.where(over, lane + float(LANES * k), 0.0))
        dropped = jnp.max(jnp.max(dropped, axis=1, keepdims=True), axis=0, keepdims=True)
        token = token[:8]
        token = jnp.where(token < float(N_TOKENS), token, jnp.broadcast_to(dropped, token.shape))
        token = token.astype(I32)
        addr_v[...] = ((token >> 3) << 5) | (token & 7)

    def filled(j, slot):
        return slot.astype(F32) < jnp.broadcast_to(total[j:j + 1], slot.shape)

    def first_expert(r0, r1):
        xs = jnp.concatenate([xg[pl.ds(r0, r1 - r0), :], jnp.zeros((8, D_IN), F32)], 0)
        y = _dot(xs, w_bufs[0][...])[:r1 - r0]
        keep = filled(0, _iota((r1 - r0, LANES), 0) + r0)
        y = [jnp.where(keep, y[:, LANES * c:LANES * (c + 1)], 0.0) for c in range(4)]
        ybuf[OWN, 0, pl.ds(r0, r1 - r0)] = _pack(y[0], y[1])
        ybuf[OWN, 1, pl.ds(r0, r1 - r0)] = _pack(y[2], y[3])

    def two_tile_pieces(j):
        xs = xg[pl.ds(SLOTS * j, SLOTS), :].astype(BF16)
        keep = filled(j, _iota((SLOTS, LANES), 0))

        def piece(p):
            w_copies[p - 1].wait()
            y = _dot(xs, w_bufs[p - 1][...])
            ybuf[OWN, p] = _pack(
                jnp.where(keep, y[:, :LANES], 0.0), jnp.where(keep, y[:, LANES:], 0.0))

        return piece

    def one_tile_pieces(j):
        rows = xg[pl.ds(SLOTS * j, SLOTS), :]
        xs = [
            [rows[m:m + 16, k:k + LANES].astype(BF16) for k in (0, LANES)]
            for m in (0, _x_row(j, 12) - SLOTS * j)
        ]
        row = _iota((16, LANES), 0)
        keep = [filled(j, row), filled(j, row + 12)]
        previous = []
        fence()

        def piece(p):
            w_copies[p - 1].wait()
            w = [w_bufs[p - 1][pl.ds(k, LANES), :].astype(BF16) for k in (0, LANES)]
            lo, hi = [
                jnp.where(ok, _dot(a[0], w[0]) + _dot(a[1], w[1]), 0.0)
                for a, ok in zip(xs, keep)
            ]
            if previous:
                lo = jnp.where(row == 12, previous.pop(), lo)
            else:
                previous.append(hi)
            block, first = _y_place(p)
            ybuf[OWN, block, pl.ds(first, _rows(p))] = _pack(lo, hi)[:_rows(p)]

        return piece

    arrived = {}

    def remote_copy(src, dst, target, group, p, r0, r1):
        block, first = _y_place(p)
        rows = pl.ds(first + r0, r1 - r0)
        recv = 3 * N_PIECES if (p, r0) == (LAST_RELAYED, CUT) else (dst - 1) * N_PIECES + p
        return pltpu.make_async_remote_copy(
            ybuf.at[src, block, rows], ybuf.at[dst, block, rows],
            send_sem.at[group], recv_sem.at[recv],
            device_id=(target,), device_id_type=mesh_id)

    def send_group(chip, route, p):
        (group,) = [
            g for g, entry in enumerate(SEND_GROUPS)
            if entry[0] == route and chip in entry[1] and p in entry[2]
        ]
        return group

    def wait_rows_from(src, p, r0, r1):
        remote_copy(OWN, src, me, 0, p, r0, r1).wait_recv()

    def send(chips, *groups):
        items = []
        for route, pieces, *rows in groups:
            for p in pieces:
                arrived.setdefault((route[0], p), set()).update(chips)
                if (route[1], p) == (DIAG, LAST_RELAYED):
                    items += [(route, p, 0, CUT), (route, p, CUT, CAP)]
                else:
                    items.append((route, p, *(rows or (0, _rows(p)))))
        items.sort(key=lambda item: item[1])

        def start():
            for route, p, r0, r1 in items:
                src, dst, to = route
                if src != OWN and r0 == 0:
                    wait_rows_from(src, p, 0, _rows(p))
                group = send_group(chips[0], route, p)
                remote_copy(src, dst, (me + to) & 3, group, p, r0, r1).start()

        on(chips, start)

    def send_to_chip0(chips, p, r0=0, r1=None):
        group = jnp.where(me == 2, 3, me - 1) if p == 0 else me - 1
        on(chips, lambda: remote_copy(OWN, me, 0, group, p, r0, r1 or _rows(p)).start())

    def pass_on(pieces):
        send((0, 3), (TO_LEFT, pieces))
        send((0, 1), (TO_RIGHT, pieces))

    def finish_sends():
        for group, (route, chips, pieces) in enumerate(SEND_GROUPS):
            block, first = _y_place(pieces[0])
            if len(pieces) == 1:
                sent = ybuf.at[route[0], block, pl.ds(first, _rows(pieces[0]))]
            else:
                blocks = pl.ds(block, _y_place(pieces[-1])[0] + 1 - block)
                sent = ybuf.at[route[0], blocks, pl.ds(0, CAP)]
            on(chips, pltpu.make_async_remote_copy(
                sent, sent, send_sem.at[group], recv_sem.at[0],
                device_id=(me,), device_id_type=mesh_id).wait_send)

    def place(src, p, r0=0, r1=None):
        r1 = r1 or _rows(p)
        if src != OWN:
            missing = tuple(c for c in range(4) if c not in arrived.get((src, p), ()))
            on(missing, lambda: wait_rows_from(src, p, r0, r1))
        j, c0, n = PIECES[p]
        block, first = _y_place(p)
        rows = [addr_s[src, SLOTS * j + s] for s in range(CAP)]

        def put(s, tile, value):
            out[pl.ds(rows[s] + 8 * tile, 1), :] = value

        for r in range(r0, r1):
            lo, hi = _unpack(ybuf[src, block, pl.ds(first + r, 1), :])
            if n == 2:
                put(r, c0, lo)
                put(r, c0 + 1, hi)
            elif r < 12:
                put(r, c0, lo)
                put(r + 12, c0, hi)
            else:
                put(24, PIECES[p - 1][1], lo)
                put(24, c0, hi)

    words = to_scalars(token_words(0))
    fence()
    later = [token_words(j) for j in (1, 2, 3)]
    for j in range(3):
        fetch_rows(j, words)
        words = to_scalars(later[j])
        fence()

    wait_rows(N_LOCAL)
    w_copies[0].wait()
    first_expert(0, EARLY)
    on((0, 1, 3), lambda: pl.semaphore_wait(barrier, 2))
    on((2,), lambda: pl.semaphore_wait(barrier, 3))
    for r0, r1 in ((0, EARLY), (EARLY, CAP)):
        if r0:
            wait_rows(0)
            first_expert(EARLY, SLOTS)
        send_to_chip0((1, 2, 3), 0, r0, r1)
        send_to_chip0((1, 3), 1, r0, r1)
        send((2,), (TO_RIGHT, (1,), r0, r1))
    pass_on((0, 1))
    fence()
    fetch_rows(3, words)
    fence()

    for p in range(2, FIRST_TILE):
        if p % 2 == 0:
            wait_rows(p // 2)
            piece = two_tile_pieces(p // 2)
        piece(p)
        send_to_chip0((1, 3), p)
        send((2,), (TO_RIGHT, (p,)))
        if p < 4:
            send((2,), (TO_LEFT, (p - 2,)))
        else:
            send((2,), (TO_LEFT, (2,), 0, 12), (TO_RIGHT, (0,)))
        pass_on((p,))
        fence()

    tiles = tuple(range(FIRST_TILE, N_PIECES))
    for p in tiles:
        if p == 5:
            piece = one_tile_pieces(2)
        if p == 7:
            wait_rows(3)
            piece = one_tile_pieces(3)
        piece(p)
        send_to_chip0((1, 2, 3), p)
        if p == 9:
            send((3,), (RELAY_RIGHT, (1,)))
        fence()
    send((2,), (TO_LEFT, (2,), 12, CAP), (TO_LEFT, range(3, N_PIECES)), (TO_RIGHT, tiles))
    pass_on(tiles)
    send((3,), (RELAY_RIGHT, (2,)))
    fence()

    build_addresses()
    addr_copy = pltpu.make_async_copy(addr_v, addr_s, misc_sem.at[1])
    addr_copy.start()
    fence()
    send((3,), (RELAY_RIGHT, (3, 4)))
    send((1,), (RELAY_RIGHT, range(N_PIECES)))
    addr_copy.wait()
    for p in range(N_PIECES):
        place(OWN, p)
    send((2,), (RELAY_RIGHT, tiles), (RELAY_LEFT, (10,)))


    for pieces in ((0, 1), (2, 3), (4,)):
        send((0,), (RELAY_RIGHT, pieces), (RELAY_LEFT, pieces))
        for src in (LEFT, RIGHT):
            for p in pieces:
                place(src, p)
        fence()
    for src, p, *rows in (
        (LEFT, 5), (LEFT, 6), (RIGHT, 5), (DIAG, 0), (RIGHT, 6), (LEFT, 7), (LEFT, 8),
        (RIGHT, 7), (LEFT, 9), (RIGHT, 8), (RIGHT, 9), (DIAG, 1), (RIGHT, 10), (LEFT, 10),
        (DIAG, 5), (DIAG, 2), (DIAG, 6), (DIAG, 7), (DIAG, 3), (DIAG, 8),
        (DIAG, LAST_RELAYED, 0, CUT), (DIAG, 9), (DIAG, LAST_RELAYED, CUT, CAP), (DIAG, 10),
    ):
        if src == LEFT and p < 10:
            send((0,), (RELAY_RIGHT, (p,)))
        if (src, p) == (DIAG, 7):
            finish_sends()
        place(src, p, *rows)


def pallas_dist_moe_cap_ep_n512_d256_e4_h512_kernel(
    x: jax.Array,
    router_W: jax.Array,
    route_idx: jax.Array,
    expert_W: jax.Array,
):
    del router_W
    in_hbm = pl.BlockSpec(memory_space=pltpu.HBM)
    tiles = D_OUT // LANES
    out = pl.pallas_call(
        _moe_kernel,
        out_shape=jax.ShapeDtypeStruct((N_TOKENS * tiles, LANES), F32),
        in_specs=[in_hbm, in_hbm, in_hbm],
        out_specs=pl.BlockSpec(memory_space=pltpu.VMEM),
        scratch_shapes=[
            pltpu.VMEM((N_TOKENS // LANES, LANES), I32),
            pltpu.VMEM((8, LANES), I32),
            pltpu.SMEM((8, LANES), I32),
            pltpu.VMEM((N_LOCAL * SLOTS, D_IN), F32),
            pltpu.VMEM((4, 2 * N_LOCAL, SLOTS, LANES), U32),
            pltpu.SemaphoreType.REGULAR,
            pltpu.SemaphoreType.DMA((2,)),
            pltpu.SemaphoreType.DMA((len(W_BLOCKS),)),
            pltpu.SemaphoreType.DMA((N_LOCAL + 1,)),
            pltpu.SemaphoreType.DMA((len(SEND_GROUPS),)),
            pltpu.SemaphoreType.DMA((3 * N_PIECES + 1,)),
            *(pltpu.VMEM((D_IN, LANES * n), F32) for _, _, n in W_BLOCKS),
        ],
        name="moe_cap_ep",
        compiler_params=pltpu.CompilerParams(
            collective_id=0, disable_bounds_checks=True, disable_semaphore_checks=True),
    )(x, route_idx.reshape(N_TOKENS // LANES, LANES), expert_W)
    out = out.reshape(N_TOKENS // 8, tiles, 8, LANES).transpose(0, 2, 1, 3)
    return out.reshape(N_TOKENS, D_OUT)
```

```python
import jax
import jax.numpy as jnp
import numpy as np
from jax import lax
from jax.experimental import pallas as pl
from jax.experimental.pallas import tpu as pltpu

F32, BF16, I32, U32 = jnp.float32, jnp.bfloat16, jnp.int32, jnp.uint32

N_TOKENS, D_IN, D_OUT = 512, 256, 512
N_EXPERTS, N_LOCAL, CAP = 16, 4, 25
LANES = 128
SLOTS = 32

OWN, RIGHT, DIAG, LEFT = 0, 1, 2, 3

PIECES = (
    (0, 0, 2), (0, 2, 2), (1, 2, 2), (1, 0, 2), (2, 0, 2),
    (2, 2, 1), (2, 3, 1), (3, 0, 1), (3, 2, 1), (3, 1, 1), (3, 3, 1),
)
N_PIECES = len(PIECES)
FIRST_TILE = 5
W_BLOCKS = ((0, 0, 4),) + PIECES[2:]
EARLY = 8
LAST_RELAYED, CUT = 4, 18

TO_LEFT = (OWN, RIGHT, LEFT)
TO_RIGHT = (OWN, LEFT, RIGHT)
TO_DIAG = (OWN, DIAG, DIAG)
RELAY_LEFT = (RIGHT, DIAG, LEFT)
RELAY_RIGHT = (LEFT, DIAG, RIGHT)

SEND_GROUPS = (
    (TO_LEFT, (0, 1, 2, 3), range(N_PIECES)),
    (TO_DIAG, (2,), range(FIRST_TILE, N_PIECES)),
    (TO_RIGHT, (0, 1, 2, 3), range(N_PIECES)),
    (TO_DIAG, (2,), range(0, 1)),
    (RELAY_RIGHT, (0,), range(0, 9)),
    (RELAY_RIGHT, (0,), range(9, 10)),
    (RELAY_LEFT, (0,), range(0, FIRST_TILE)),
    (RELAY_RIGHT, (1,), range(N_PIECES)),
    (RELAY_RIGHT, (2,), range(FIRST_TILE, N_PIECES)),
    (RELAY_LEFT, (2,), range(10, 11)),
    (RELAY_RIGHT, (3,), range(1, FIRST_TILE)),
)


def _rows(p):
    return CAP if p < FIRST_TILE else 12 + (p - FIRST_TILE) % 2


def _y_place(p):
    if p < FIRST_TILE:
        return p, 0
    return FIRST_TILE + (p - FIRST_TILE) // 2, (13 if _rows(p) == 12 else 0)


def _x_row(j, s):
    return SLOTS * j + (s + 4 if j == N_LOCAL - 1 and s >= 12 else s)


def _iota(shape, axis):
    return lax.broadcasted_iota(I32, shape, axis)


def _dot(a, b):
    return jnp.dot(a.astype(BF16), b.astype(BF16), preferred_element_type=F32)


def _pack(lo, hi):
    lo, hi = (lax.bitcast_convert_type(v.astype(BF16).astype(F32), U32) for v in (lo, hi))
    return (lo >> 16) | (hi & np.uint32(0xFFFF0000))


def _unpack(words):
    lo, hi = words << 16, words & np.uint32(0xFFFF0000)
    return lax.bitcast_convert_type(lo, F32), lax.bitcast_convert_type(hi, F32)


def _moe_kernel(x_hbm, route_hbm, w_hbm, out, route, addr_v, addr_s, xg, ybuf,
                fence_sem, misc_sem, w_sem, x_sem, send_sem, recv_sem, *w_bufs):

    def fence():
        pl.semaphore_signal(fence_sem, 1)
        pl.semaphore_wait(fence_sem, 1)

    route_copy = pltpu.make_async_copy(route_hbm, route, misc_sem.at[0])
    route_copy.start()
    fence()
    w_copies = []
    for i, (j, c0, n) in enumerate(W_BLOCKS):
        src = w_hbm.at[j] if n == 4 else w_hbm.at[j, :, pl.ds(LANES * c0, LANES * n)]
        w_copies.append(pltpu.make_async_copy(src, w_bufs[i], w_sem.at[i]))
        w_copies[i].start(priority=1)
    fence()

    me = lax.axis_index("i")
    mesh_id = pl.DeviceIdType.MESH

    def on(chips, fn):
        if len(chips) == 4:
            fn()
        elif len(chips) == 3:
            pl.when(me != 6 - sum(chips))(fn)
        elif chips:
            pl.when(((sum(1 << c for c in chips) >> me) & 1) == 1)(fn)

    barrier = pltpu.get_barrier_semaphore()

    def tell(distance):
        pl.semaphore_signal(barrier, 1, device_id=((me + distance) & 3,), device_id_type=mesh_id)

    tell(RIGHT)
    tell(LEFT)
    on((0,), lambda: tell(DIAG))

    for row in (24, 56, 88, 104, 120):
        xg[pl.ds(row, 8), :] = jnp.zeros((8, D_IN), F32)
    out[...] = jnp.zeros(out.shape, F32)

    def running_counts(n):
        expert = (_iota((n, LANES), 0) + N_LOCAL * me) & (N_EXPERTS - 1)
        hit = [
            jnp.broadcast_to(route[pl.ds(k, 1), :] & (N_EXPERTS - 1), (n, LANES)) == expert
            for k in range(4)
        ]
        flags = [jnp.where(h, 1.0, 0.0) for h in hit]
        earlier = [flags[0]]
        for k in range(1, 4):
            earlier.append(earlier[-1] + flags[k])
        square = (LANES, LANES)
        upto = jnp.where(_iota(square, 0) <= _iota(square, 1), 1.0, 0.0)
        ones = jnp.ones(square, BF16)
        a = [_dot(jnp.concatenate(flags[k:k + 2], 0), upto) for k in (0, 2)]
        b = [_dot(jnp.concatenate(earlier[k:k + 2], 0), ones) for k in (0, 2)]
        counts = [a[0][:n], a[0][n:] + b[0][:n], a[1][:n] + b[0][n:], a[1][n:] + b[1][:n]]
        return hit, counts, b[1][n:]

    route_copy.wait()
    _, counts, total = running_counts(8)

    def token_words(j):
        shape = (16, LANES)
        even = 2.0 * _iota(shape, 0).astype(F32)
        acc = None
        for k in range(4):
            c = jnp.broadcast_to(counts[k][j:j + 1], shape)
            both, odd_only, none = 1025.0, 1024.0, 0.0
            if k == 0:
                both, odd_only, none = both + 65536.0, odd_only + 65536.0, 65536.0
            if k == 3:
                last = _iota(shape, 1) == LANES - 1
                both, odd_only = jnp.where(last, 0.0, both), jnp.where(last, 0.0, odd_only)
            v = jnp.where(c <= even, both, jnp.where(c <= even + 1.0, odd_only, none))
            acc = v if acc is None else acc + v
        acc = jnp.broadcast_to(jnp.sum(acc, axis=1, keepdims=True), shape)
        return lax.bitcast_convert_type(acc, I32) & 0xFFFFF

    def to_scalars(words):
        return [words[r, 0] for r in range((CAP + 1) // 2)]

    row_copies = {}

    def fetch_rows(j, words):
        for s in range(CAP):
            token = words[s // 2] >> 10 if s & 1 else words[s // 2] & 1023
            group = N_LOCAL if j == 0 and s < EARLY else j
            copy = pltpu.make_async_copy(
                x_hbm.at[pl.ds(token, 1)], xg.at[pl.ds(_x_row(j, s), 1)], x_sem.at[group])
            copy.start()
            row_copies.setdefault(group, []).append(copy)
            if s in (7, 15):
                fence()

    def wait_rows(group):
        for copy in row_copies[group]:
            copy.wait()

    def build_addresses():
        hit, counts, _ = running_counts(N_EXPERTS)
        slot = _iota((SLOTS, LANES), 0).astype(F32)
        token = None
        for d in range(4):
            parts = []
            for e in range(N_LOCAL * d, N_LOCAL * (d + 1)):
                below = [
                    jnp.where(jnp.broadcast_to(c[e:e + 1], slot.shape) <= slot, 1.0, 0.0)
                    for c in counts
                ]
                parts.append((below[0] + below[1]) + (below[2] + below[3]))
            t = lax.dot_general(
                jnp.where(_iota((16, LANES), 0) == d, 1.0, 0.0).astype(BF16),
                jnp.concatenate(parts, 0).astype(BF16),
                (((1,), (1,)), ((), ())), preferred_element_type=F32)
            token = t if token is None else token + t
        lane = _iota((N_EXPERTS, LANES), 1).astype(F32)
        dropped = jnp.zeros_like(lane)
        for k in range(4):
            over = hit[k] & (counts[k] > float(CAP))
            dropped = jnp.maximum(dropped, jnp.where(over, lane + float(LANES * k), 0.0))
        dropped = jnp.max(jnp.max(dropped, axis=1, keepdims=True), axis=0, keepdims=True)
        token = token[:8]
        token = jnp.where(token < float(N_TOKENS), token, jnp.broadcast_to(dropped, token.shape))
        token = token.astype(I32)
        addr_v[...] = ((token >> 3) << 5) | (token & 7)

    def filled(j, slot):
        return slot.astype(F32) < jnp.broadcast_to(total[j:j + 1], slot.shape)

    def first_expert(r0, r1):
        xs = jnp.concatenate([xg[pl.ds(r0, r1 - r0), :], jnp.zeros((8, D_IN), F32)], 0)
        y = _dot(xs, w_bufs[0][...])[:r1 - r0]
        keep = filled(0, _iota((r1 - r0, LANES), 0) + r0)
        y = [jnp.where(keep, y[:, LANES * c:LANES * (c + 1)], 0.0) for c in range(4)]
        ybuf[OWN, 0, pl.ds(r0, r1 - r0)] = _pack(y[0], y[1])
        ybuf[OWN, 1, pl.ds(r0, r1 - r0)] = _pack(y[2], y[3])

    def two_tile_pieces(j):
        xs = xg[pl.ds(SLOTS * j, SLOTS), :].astype(BF16)
        keep = filled(j, _iota((SLOTS, LANES), 0))

        def piece(p):
            w_copies[p - 1].wait()
            y = _dot(xs, w_bufs[p - 1][...])
            ybuf[OWN, p] = _pack(
                jnp.where(keep, y[:, :LANES], 0.0), jnp.where(keep, y[:, LANES:], 0.0))

        return piece

    def one_tile_pieces(j):
        rows = xg[pl.ds(SLOTS * j, SLOTS), :]
        xs = [
            [rows[m:m + 16, k:k + LANES].astype(BF16) for k in (0, LANES)]
            for m in (0, _x_row(j, 12) - SLOTS * j)
        ]
        row = _iota((16, LANES), 0)
        keep = [filled(j, row), filled(j, row + 12)]
        previous = []
        fence()

        def piece(p):
            w_copies[p - 1].wait()
            w = [w_bufs[p - 1][pl.ds(k, LANES), :].astype(BF16) for k in (0, LANES)]
            lo, hi = [
                jnp.where(ok, _dot(a[0], w[0]) + _dot(a[1], w[1]), 0.0)
                for a, ok in zip(xs, keep)
            ]
            if previous:
                lo = jnp.where(row == 12, previous.pop(), lo)
            else:
                previous.append(hi)
            block, first = _y_place(p)
            ybuf[OWN, block, pl.ds(first, _rows(p))] = _pack(lo, hi)[:_rows(p)]

        return piece

    arrived = {}

    def remote_copy(src, dst, target, group, p, r0, r1):
        block, first = _y_place(p)
        rows = pl.ds(first + r0, r1 - r0)
        recv = 3 * N_PIECES if (p, r0) == (LAST_RELAYED, CUT) else (dst - 1) * N_PIECES + p
        return pltpu.make_async_remote_copy(
            ybuf.at[src, block, rows], ybuf.at[dst, block, rows],
            send_sem.at[group], recv_sem.at[recv],
            device_id=(target,), device_id_type=mesh_id)

    def send_group(chip, route, p):
        (group,) = [
            g for g, entry in enumerate(SEND_GROUPS)
            if entry[0] == route and chip in entry[1] and p in entry[2]
        ]
        return group

    def wait_rows_from(src, p, r0, r1):
        remote_copy(OWN, src, me, 0, p, r0, r1).wait_recv()

    def send(chips, *groups):
        items = []
        for route, pieces, *rows in groups:
            for p in pieces:
                arrived.setdefault((route[0], p), set()).update(chips)
                if (route[1], p) == (DIAG, LAST_RELAYED):
                    items += [(route, p, 0, CUT), (route, p, CUT, CAP)]
                else:
                    items.append((route, p, *(rows or (0, _rows(p)))))
        items.sort(key=lambda item: item[1])

        def start():
            for route, p, r0, r1 in items:
                src, dst, to = route
                if src != OWN and r0 == 0:
                    wait_rows_from(src, p, 0, _rows(p))
                group = send_group(chips[0], route, p)
                remote_copy(src, dst, (me + to) & 3, group, p, r0, r1).start()

        on(chips, start)

    def send_to_chip0(chips, p, r0=0, r1=None):
        group = jnp.where(me == 2, 3, me - 1) if p == 0 else me - 1
        on(chips, lambda: remote_copy(OWN, me, 0, group, p, r0, r1 or _rows(p)).start())

    def pass_on(pieces):
        send((0, 3), (TO_LEFT, pieces))
        send((0, 1), (TO_RIGHT, pieces))

    def finish_sends():
        for group, (route, chips, pieces) in enumerate(SEND_GROUPS):
            block, first = _y_place(pieces[0])
            if len(pieces) == 1:
                sent = ybuf.at[route[0], block, pl.ds(first, _rows(pieces[0]))]
            else:
                blocks = pl.ds(block, _y_place(pieces[-1])[0] + 1 - block)
                sent = ybuf.at[route[0], blocks, pl.ds(0, CAP)]
            on(chips, pltpu.make_async_remote_copy(
                sent, sent, send_sem.at[group], recv_sem.at[0],
                device_id=(me,), device_id_type=mesh_id).wait_send)

    def place(src, p, r0=0, r1=None):
        r1 = r1 or _rows(p)
        if src != OWN:
            missing = tuple(c for c in range(4) if c not in arrived.get((src, p), ()))
            on(missing, lambda: wait_rows_from(src, p, r0, r1))
        j, c0, n = PIECES[p]
        block, first = _y_place(p)
        rows = [addr_s[src, SLOTS * j + s] for s in range(CAP)]

        def put(s, tile, value):
            out[pl.ds(rows[s] + 8 * tile, 1), :] = value

        for r in range(r0, r1):
            lo, hi = _unpack(ybuf[src, block, pl.ds(first + r, 1), :])
            if n == 2:
                put(r, c0, lo)
                put(r, c0 + 1, hi)
            elif r < 12:
                put(r, c0, lo)
                put(r + 12, c0, hi)
            else:
                put(24, PIECES[p - 1][1], lo)
                put(24, c0, hi)

    words = to_scalars(token_words(0))
    fence()
    later = [token_words(j) for j in (1, 2, 3)]
    for j in range(3):
        fetch_rows(j, words)
        words = to_scalars(later[j])
        fence()

    wait_rows(N_LOCAL)
    w_copies[0].wait()
    first_expert(0, EARLY)
    on((0, 1, 3), lambda: pl.semaphore_wait(barrier, 2))
    on((2,), lambda: pl.semaphore_wait(barrier, 3))
    for r0, r1 in ((0, EARLY), (EARLY, CAP)):
        if r0:
            wait_rows(0)
            first_expert(EARLY, SLOTS)
        send_to_chip0((1, 2, 3), 0, r0, r1)
        send_to_chip0((1, 3), 1, r0, r1)
        send((2,), (TO_RIGHT, (1,), r0, r1))
    pass_on((0, 1))
    fence()
    fetch_rows(3, words)
    fence()

    for p in range(2, FIRST_TILE):
        if p % 2 == 0:
            wait_rows(p // 2)
            piece = two_tile_pieces(p // 2)
        piece(p)
        send_to_chip0((1, 3), p)
        send((2,), (TO_RIGHT, (p,)))
        if p < 4:
            send((2,), (TO_LEFT, (p - 2,)))
        else:
            send((2,), (TO_LEFT, (2,), 0, 12), (TO_RIGHT, (0,)))
        pass_on((p,))
        fence()

    tiles = tuple(range(FIRST_TILE, N_PIECES))
    for p in tiles:
        if p == 5:
            piece = one_tile_pieces(2)
        if p == 7:
            wait_rows(3)
            piece = one_tile_pieces(3)
        piece(p)
        send_to_chip0((1, 2, 3), p)
        if p == 5:
            send((1,), (RELAY_RIGHT, (0,)))
        if p == 9:
            send((3,), (RELAY_RIGHT, (1,)))
        fence()
    send((2,), (TO_LEFT, (2,), 12, CAP), (TO_LEFT, range(3, N_PIECES)), (TO_RIGHT, tiles))
    pass_on(tiles)
    send((3,), (RELAY_RIGHT, (2,)))
    fence()

    build_addresses()
    addr_copy = pltpu.make_async_copy(addr_v, addr_s, misc_sem.at[1])
    addr_copy.start()
    fence()
    send((3,), (RELAY_RIGHT, (3, 4)))
    send((1,), (RELAY_RIGHT, range(1, N_PIECES)))
    send((2,), (RELAY_RIGHT, tiles), (RELAY_LEFT, (10,)))
    addr_copy.wait()
    for p in range(N_PIECES):
        place(OWN, p)

    for pieces in ((0, 1), (2, 3), (4,)):
        send((0,), (RELAY_RIGHT, pieces), (RELAY_LEFT, pieces))
        for src in (LEFT, RIGHT):
            for p in pieces:
                place(src, p)
        fence()
    for src, p, *rows in (
        (LEFT, 5), (LEFT, 6), (RIGHT, 5), (DIAG, 0), (RIGHT, 6), (LEFT, 7), (LEFT, 8),
        (RIGHT, 7), (LEFT, 9), (RIGHT, 8), (RIGHT, 9), (DIAG, 1), (RIGHT, 10), (LEFT, 10),
        (DIAG, 5), (DIAG, 2), (DIAG, 6), (DIAG, 7), (DIAG, 3), (DIAG, 8),
        (DIAG, LAST_RELAYED, 0, CUT), (DIAG, 9), (DIAG, LAST_RELAYED, CUT, CAP), (DIAG, 10),
    ):
        if src == LEFT and p < 10:
            send((0,), (RELAY_RIGHT, (p,)))
        if (src, p) == (DIAG, 7):
            finish_sends()
        place(src, p, *rows)


def pallas_dist_moe_cap_ep_n512_d256_e4_h512_kernel(
    x: jax.Array,
    router_W: jax.Array,
    route_idx: jax.Array,
    expert_W: jax.Array,
):
    del router_W
    in_hbm = pl.BlockSpec(memory_space=pltpu.HBM)
    tiles = D_OUT // LANES
    out = pl.pallas_call(
        _moe_kernel,
        out_shape=jax.ShapeDtypeStruct((N_TOKENS * tiles, LANES), F32),
        in_specs=[in_hbm, in_hbm, in_hbm],
        out_specs=pl.BlockSpec(memory_space=pltpu.VMEM),
        scratch_shapes=[
            pltpu.VMEM((N_TOKENS // LANES, LANES), I32),
            pltpu.VMEM((8, LANES), I32),
            pltpu.SMEM((8, LANES), I32),
            pltpu.VMEM((N_LOCAL * SLOTS, D_IN), F32),
            pltpu.VMEM((4, 2 * N_LOCAL, SLOTS, LANES), U32),
            pltpu.SemaphoreType.REGULAR,
            pltpu.SemaphoreType.DMA((2,)),
            pltpu.SemaphoreType.DMA((len(W_BLOCKS),)),
            pltpu.SemaphoreType.DMA((N_LOCAL + 1,)),
            pltpu.SemaphoreType.DMA((len(SEND_GROUPS),)),
            pltpu.SemaphoreType.DMA((3 * N_PIECES + 1,)),
            *(pltpu.VMEM((D_IN, LANES * n), F32) for _, _, n in W_BLOCKS),
        ],
        name="moe_cap_ep",
        compiler_params=pltpu.CompilerParams(
            collective_id=0, disable_bounds_checks=True, disable_semaphore_checks=True),
    )(x, route_idx.reshape(N_TOKENS // LANES, LANES), expert_W)
    out = out.reshape(N_TOKENS // 8, tiles, 8, LANES).transpose(0, 2, 1, 3)
    return out.reshape(N_TOKENS, D_OUT)
```
